```python
import numpy as np

kernel_name = "dist_moe_shared_ep_outshard_n256_d128_e2_h256"

def setup_inputs():
    x = np.random.randn(256, 128).astype(np.float32)
    router_W = np.random.randn(128, 8).astype(np.float32) * 0.1
    scores64 = x.astype(np.float64) @ router_W.astype(np.float64)
    route_idx = np.argsort(-scores64, axis=-1)[:, :1].astype(np.int32)
    expert_W = np.random.randn(8, 128, 256).astype(np.float32) * 0.02
    shared_W = np.random.randn(128, 256).astype(np.float32) * 0.02
    return {"x": x, "router_W": router_W, "route_idx": route_idx, "expert_W": expert_W, "shared_W": shared_W}

def reference(x, router_W, route_idx, expert_W, shared_W):
    scores = x @ router_W
    s_max = scores.max(axis=-1, keepdims=True)
    probs = np.exp(scores - s_max)
    probs = probs / probs.sum(axis=-1, keepdims=True)
    shared = x @ shared_W
    out = np.zeros((256, 256), dtype=np.float32)
    for i in range(256):
        e = int(route_idx[i, 0])
        out[i] = shared[i] + probs[i, e] * (x[i] @ expert_W[e])
    return out
```

```python
import jax
import jax.numpy as jnp
from jax import lax
from jax.experimental import pallas as pl
from jax.experimental.pallas import tpu as pltpu

N_DEV = 4
N, D, H, E = 256, 128, 256, 8
NB = N // N_DEV
R = 32
HH = H // 2
F32, BF16, I32 = jnp.float32, jnp.bfloat16, jnp.int32
LATE = 2


def _dot(a, b):
    return jnp.dot(a, b, preferred_element_type=F32)


def pallas_dist_moe_shared_ep_outshard_n256_d128_e2_h256_kernel(x, router_W, route_idx, expert_W, shared_W):
    def body(x_hbm, rwt_hbm, idx_hbm, ew_hbm, sw_hbm, out_ref,
             x_v, rwt_v, idx_v, ew_v, sw_v, acc_v, ybuf, rbuf, ybuf1, rbuf1,
             lsem, send_sems, recv_sems):
        cp_idx = pltpu.make_async_copy(idx_hbm, idx_v, lsem.at[0])
        cp_x0 = pltpu.make_async_copy(x_hbm.at[pl.ds(0, NB)], x_v.at[pl.ds(0, NB)], lsem.at[1])
        cp_w = [pltpu.make_async_copy(ew_hbm.at[:, :, pl.ds(h * HH, HH)], ew_v.at[h], lsem.at[2 + h]) for h in range(2)]
        cp_xr = pltpu.make_async_copy(x_hbm.at[pl.ds(NB, N - NB)], x_v.at[pl.ds(NB, N - NB)], lsem.at[4])
        cp_sw = pltpu.make_async_copy(sw_hbm, sw_v, lsem.at[5])
        cp_rw = pltpu.make_async_copy(rwt_hbm, rwt_v, lsem.at[6])
        cp_idx.start()
        cp_x0.start()
        cp_w[0].start()
        cp_w[1].start()

        me = lax.axis_index("i")
        barrier = pltpu.get_barrier_semaphore()
        for d in (2, 1, 3):
            pl.semaphore_signal(barrier, inc=1, device_id=((me + d) % N_DEV,), device_id_type=pl.DeviceIdType.MESH)
        cp_xr.start()
        cp_sw.start()
        cp_rw.start()

        def rdma(j, h, slot):
            return pltpu.make_async_remote_copy(
                src_ref=ybuf.at[j, h], dst_ref=rbuf.at[slot, h],
                send_sem=send_sems.at[2 * j + h], recv_sem=recv_sems.at[2 * slot + h],
                device_id=(j,), device_id_type=pl.DeviceIdType.MESH)

        def rdma1(j, slot):
            return pltpu.make_async_remote_copy(
                src_ref=ybuf1.at[j], dst_ref=rbuf1.at[slot],
                send_sem=send_sems.at[8 + j], recv_sem=recv_sems.at[8 + slot],
                device_id=(j,), device_id_type=pl.DeviceIdType.MESH)

        ui = lax.broadcasted_iota(I32, (128, 128), 0)
        uj = lax.broadcasted_iota(I32, (128, 128), 1)
        tri = ((ui < uj) & ((ui ^ uj) < NB)).astype(BF16)
        sub8 = lax.broadcasted_iota(I32, (8, 128), 0)
        lane1 = lax.broadcasted_iota(I32, (1, 128), 1)
        hi = lane1 >= NB
        row_f = ui.astype(F32)

        cp_idx.wait()
        idx_a = idx_v[0:1, :]
        idx_b = idx_v[1:2, :]
        idx8 = jnp.where(sub8 < 4, idx_a, idx_b)
        oh = (idx8 >> 1) == (sub8 & 3)
        cum = _dot(oh.astype(BF16), tri)
        rk = jnp.where(oh, cum, 0.0)
        rank = [jnp.sum(rk[0:4], axis=0, keepdims=True), jnp.sum(rk[4:8], axis=0, keepdims=True)]
        idxs = [idx_a, idx_b]
        mine = [(t >> 1) == me for t in idxs]
        second = [(t & 1) == 1 for t in idxs]

        s0 = jnp.where(mine[0] & (rank[0] < R), rank[0] + jnp.where(second[0], float(R), 0.0), -1.0)
        pp0 = (row_f[:2 * R, :NB] == s0[:, :NB]).astype(BF16)
        cp_x0.wait()
        x0 = x_v[0:NB, :].astype(BF16)
        xa0 = _dot(pp0[:R], x0).astype(BF16)
        xb0 = _dot(pp0[R:], x0).astype(BF16)

        @pl.when(me == LATE)
        def _():
            pl.semaphore_wait(barrier, N_DEV - 1)

        ws = []
        for h in range(2):
            cp_w[h].wait()
            ws.append((ew_v[h, 0].astype(BF16), ew_v[h, 1].astype(BF16)))
            ybuf[0, h] = (_dot(xa0, ws[h][0]) + _dot(xb0, ws[h][1])).astype(BF16)

            @pl.when(me == LATE)
            def _():
                rdma(0, h, me).start()

        pp1 = (row_f[:2 * R] == jnp.where(hi, s0, -1.0)).astype(BF16)
        s1 = jnp.where(mine[1] & (rank[1] < R),
                       rank[1] + jnp.where(second[1], float(2 * R), 0.0) + jnp.where(hi, float(R), 0.0), -1.0)
        pp23 = (row_f == s1).astype(BF16)
        cp_xr.wait()
        xlo = x_v[0:128, :].astype(BF16)
        xhi = x_v[128:256, :].astype(BF16)
        xc1 = _dot(pp1, xlo).astype(BF16)
        xc23 = _dot(pp23, xhi).astype(BF16)
        xa = jnp.concatenate([xc1[:R], xc23[:2 * R]], axis=0)
        xb = jnp.concatenate([xc1[R:], xc23[2 * R:]], axis=0)
        for h in range(2):
            y = (_dot(xa, ws[h][0]) + _dot(xb, ws[h][1])).astype(BF16)
            for j in range(1, 4):
                ybuf[j, h] = y[(j - 1) * R:j * R]

        @pl.when(me != LATE)
        def _():
            pl.semaphore_wait(barrier, N_DEV - 1)

            @pl.when(me != 0)
            def _():
                for h in range(2):
                    rdma(0, h, me).start()

        for j in range(1, 4):
            @pl.when(me != j)
            def _():
                for h in range(2):
                    rdma(j, h, me).start()

        low = me < 2
        my_idx = jnp.where(low, idx_a, idx_b)
        my_rank = jnp.where(low, rank[0], rank[1])
        xh = jnp.where(low, xlo, xhi)
        cp_rw.wait()
        sc = lax.dot_general(rwt_v[...].astype(BF16), xh, (((1,), (1,)), ((), ())), preferred_element_type=F32)
        pe = jnp.exp(sc - jnp.max(sc, axis=0, keepdims=True))
        gate_row = jnp.sum(jnp.where(sub8 == my_idx, pe, 0.0), axis=0, keepdims=True) / jnp.sum(pe, axis=0, keepdims=True)
        g_row = (my_idx >> 1).astype(F32) * float(NB) + my_rank
        pick = uj[:NB] == ui[:NB] + (me % 2) * NB
        g_col = jnp.sum(jnp.where(pick, g_row, 0.0), axis=1, keepdims=True)
        gate = jnp.sum(jnp.where(pick, gate_row, 0.0), axis=1, keepdims=True)
        overflow = jnp.max(jnp.maximum(rank[0], rank[1])) >= float(R)
        k1, k2, k3 = (me + 1) % N_DEV, (me + 2) % N_DEV, (me + 3) % N_DEV
        c = lane1[:, :3 * R]
        tgt3 = jnp.where(c < R, me * NB + c, jnp.where(c < 2 * R, k1 * NB + c - R, k3 * NB + c - 2 * R)).astype(F32)
        pt3 = (g_col == tgt3).astype(BF16)
        pt_last = (g_col == (k2 * NB + lane1[:, :R]).astype(F32)).astype(BF16)
        xm = x_v[pl.ds(pl.multiple_of(me * NB, NB), NB), :].astype(BF16)
        cp_sw.wait()
        acc_v[...] = _dot(xm, sw_v[...].astype(BF16))

        @pl.when(overflow)
        def _():
            pps = []
            for t in range(2):
                st = jnp.where(mine[t] & (rank[t] >= R),
                               rank[t] - float(R) + jnp.where(second[t], float(2 * R), 0.0) + jnp.where(hi, float(R), 0.0), -1.0)
                pps.append((row_f == st).astype(BF16))
            c01 = _dot(pps[0], xlo).astype(BF16)
            c23 = _dot(pps[1], xhi).astype(BF16)
            oa = jnp.concatenate([c01[:2 * R], c23[:2 * R]], axis=0)
            ob = jnp.concatenate([c01[2 * R:], c23[2 * R:]], axis=0)
            for h in range(2):
                y = (_dot(oa, ew_v[h, 0].astype(BF16)) + _dot(ob, ew_v[h, 1].astype(BF16))).astype(BF16)
                for j in range(N_DEV):
                    ybuf1[j, :, h * HH:(h + 1) * HH] = y[j * R:(j + 1) * R]
            for j in range(N_DEV):
                @pl.when(me != j)
                def _():
                    rdma1(j, me).start()
            rbuf1[me] = ybuf1[me]
            for k in (k1, k2, k3):
                rdma1(k, k).wait_recv()
            tgt = ((lane1 >> 5) * NB + (lane1 & (R - 1)) + R).astype(F32)
            ptf = (g_col == tgt).astype(BF16)
            yall = jnp.concatenate([rbuf1[k] for k in range(N_DEV)], axis=0)
            acc_v[...] += gate * _dot(ptf, yall)
            for k in (k1, k2, k3):
                rdma1(k, k).wait_send()

        for k in (k1, k3):
            for h in range(2):
                rdma(k, h, k).wait_recv()
        base = []
        for h in range(2):
            y3 = jnp.concatenate([ybuf[me, h], rbuf[k1, h], rbuf[k3, h]], axis=0)
            base.append(acc_v[:, h * HH:(h + 1) * HH] + gate * _dot(pt3, y3))
        for k in (k1, k2, k3):
            for h in range(2):
                rdma(k, h, k).wait_send()
        for h in range(2):
            rdma(k2, h, k2).wait_recv()
            yl = rbuf[k2, h]
            for m in range(2):
                sl = slice(m * R, (m + 1) * R)
                out_ref[sl, h * HH:(h + 1) * HH] = base[h][sl] + gate[sl] * _dot(pt_last[sl], yl)

    return pl.pallas_call(
        body,
        out_shape=jax.ShapeDtypeStruct((NB, H), F32),
        in_specs=[pl.BlockSpec(memory_space=pl.ANY)] * 5,
        out_specs=pl.BlockSpec(memory_space=pltpu.VMEM),
        scratch_shapes=[
            pltpu.VMEM((N, D), F32),
            pltpu.VMEM((E, D), F32),
            pltpu.VMEM((2, 128), I32),
            pltpu.VMEM((2, 2, D, HH), F32),
            pltpu.VMEM((D, H), F32),
            pltpu.VMEM((NB, H), F32),
            pltpu.VMEM((N_DEV, 2, R, HH), BF16),
            pltpu.VMEM((N_DEV, 2, R, HH), BF16),
            pltpu.VMEM((N_DEV, R, H), BF16),
            pltpu.VMEM((N_DEV, R, H), BF16),
            pltpu.SemaphoreType.DMA((7,)),
            pltpu.SemaphoreType.DMA((12,)),
            pltpu.SemaphoreType.DMA((12,)),
        ],
        compiler_params=pltpu.CompilerParams(collective_id=0, disable_bounds_checks=True, disable_semaphore_checks=True),
    )(x, router_W.T, route_idx.reshape(2, 128), expert_W, shared_W)
```

```python
import jax
import jax.numpy as jnp
from jax import lax
from jax.experimental import pallas as pl
from jax.experimental.pallas import tpu as pltpu

N_DEV = 4
N, D, H, E = 256, 128, 256, 8
NB = N // N_DEV
R = 32
RW = R // 2
HH = H // 2
F32, BF16, I32, U32 = jnp.float32, jnp.bfloat16, jnp.int32, jnp.uint32
LATE = 2


def _dot(a, b):
    return jnp.dot(a, b, preferred_element_type=F32)


def pallas_dist_moe_shared_ep_outshard_n256_d128_e2_h256_kernel(x, router_W, route_idx, expert_W, shared_W):
    def body(x_hbm, rwt_hbm, idx_hbm, ew_hbm, sw_hbm, out_ref,
             x_v, rwt_v, idx_v, ew_v, sw_v, acc_v, ybuf, rbuf, ybuf1, rbuf1,
             lsem, send_sems, recv_sems):
        cp_idx = pltpu.make_async_copy(idx_hbm, idx_v, lsem.at[0])
        cp_x0 = pltpu.make_async_copy(x_hbm.at[pl.ds(0, NB)], x_v.at[pl.ds(0, NB)], lsem.at[1])
        cp_w = [pltpu.make_async_copy(ew_hbm.at[:, :, pl.ds(h * HH, HH)], ew_v.at[h], lsem.at[2 + h]) for h in range(2)]
        cp_xr = pltpu.make_async_copy(x_hbm.at[pl.ds(NB, N - NB)], x_v.at[pl.ds(NB, N - NB)], lsem.at[4])
        cp_sw = pltpu.make_async_copy(sw_hbm, sw_v, lsem.at[5])
        cp_rw = pltpu.make_async_copy(rwt_hbm, rwt_v, lsem.at[6])
        cp_idx.start()
        cp_x0.start()
        cp_w[0].start()
        cp_w[1].start()

        me = lax.axis_index("i")
        barrier = pltpu.get_barrier_semaphore()
        for d in (2, 1, 3):
            pl.semaphore_signal(barrier, inc=1, device_id=((me + d) % N_DEV,), device_id_type=pl.DeviceIdType.MESH)
        cp_xr.start()
        cp_sw.start()
        cp_rw.start()

        def rdma(j, h, slot, m):
            return pltpu.make_async_remote_copy(
                src_ref=ybuf.at[j, h, pl.ds(0, m)], dst_ref=rbuf.at[slot, h, pl.ds(0, m)],
                send_sem=send_sems.at[2 * j + h], recv_sem=recv_sems.at[2 * slot + h],
                device_id=(j,), device_id_type=pl.DeviceIdType.MESH)

        def rdma1(j, slot):
            return pltpu.make_async_remote_copy(
                src_ref=ybuf1.at[j], dst_ref=rbuf1.at[slot],
                send_sem=send_sems.at[8 + j], recv_sem=recv_sems.at[8 + slot],
                device_id=(j,), device_id_type=pl.DeviceIdType.MESH)

        ui = lax.broadcasted_iota(I32, (128, 128), 0)
        uj = lax.broadcasted_iota(I32, (128, 128), 1)
        tri = (((ui < uj) & ((ui ^ uj) < NB)) | (uj == 0)).astype(BF16)
        sub8 = lax.broadcasted_iota(I32, (8, 128), 0)
        sub16 = ui[:16]
        lane1 = lax.broadcasted_iota(I32, (1, 128), 1)
        hi = lane1 >= NB
        row_f = ui.astype(F32)

        cp_idx.wait()
        idx_a = idx_v[0:1, :]
        idx_b = idx_v[1:2, :]
        idx16 = jnp.where(sub16 < 8, idx_a, idx_b)
        oh = ((idx16 >> 1) == (sub16 & 3)) & (hi == ((sub16 & 4) != 0))
        cum = _dot(oh.astype(BF16), tri)
        rk = jnp.where(oh & (lane1 > 0), cum, 0.0)
        rank = [jnp.sum(rk[0:8], axis=0, keepdims=True), jnp.sum(rk[8:16], axis=0, keepdims=True)]
        idxs = [idx_a, idx_b]
        mine = [(t >> 1) == me for t in idxs]
        second = [(t & 1) == 1 for t in idxs]

        def words(b, c):
            n = jnp.sum(jnp.where(sub16 == 4 * b + c, cum, 0.0), axis=0, keepdims=True).astype(I32)
            return jnp.clip((n[0, 0] + 1) >> 1, 1, RW)

        s0 = jnp.where(mine[0] & (rank[0] < R), rank[0] + jnp.where(second[0], float(R), 0.0), -1.0)
        pp0 = (row_f[:2 * R, :NB] == s0[:, :NB]).astype(BF16)
        cp_x0.wait()
        x0 = x_v[0:NB, :].astype(BF16)
        xq = [_dot(pp0[q * 16:(q + 1) * 16], x0).astype(BF16) for q in range(4)]
        m_send = [words(j, me) for j in range(N_DEV)]

        @pl.when(me == LATE)
        def _():
            pl.semaphore_wait(barrier, N_DEV - 1)

        ws = []
        for h in range(2):
            cp_w[h].wait()
            ws.append((ew_v[h, 0].astype(BF16), ew_v[h, 1].astype(BF16)))
            for q in range(2):
                yq = (_dot(xq[q], ws[h][0]) + _dot(xq[2 + q], ws[h][1])).astype(BF16)
                ybuf[0, h, q * 8:(q + 1) * 8, :] = pltpu.bitcast(yq, U32)

            @pl.when(me == LATE)
            def _():
                rdma(0, h, me, m_send[0]).start()

        pp1 = (row_f[:2 * R] == jnp.where(hi, s0, -1.0)).astype(BF16)
        s1 = jnp.where(mine[1] & (rank[1] < R),
                       rank[1] + jnp.where(second[1], float(2 * R), 0.0) + jnp.where(hi, float(R), 0.0), -1.0)
        pp23 = (row_f == s1).astype(BF16)
        cp_xr.wait()
        xlo = x_v[0:128, :].astype(BF16)
        xhi = x_v[128:256, :].astype(BF16)
        xc1 = _dot(pp1, xlo).astype(BF16)
        xc23 = _dot(pp23, xhi).astype(BF16)
        xa = jnp.concatenate([xc1[:R], xc23[:2 * R]], axis=0)
        xb = jnp.concatenate([xc1[R:], xc23[2 * R:]], axis=0)
        for h in range(2):
            y = pltpu.bitcast((_dot(xa, ws[h][0]) + _dot(xb, ws[h][1])).astype(BF16), U32)
            for j in range(1, 4):
                ybuf[j, h] = y[(j - 1) * RW:j * RW]

        @pl.when(me != LATE)
        def _():
            pl.semaphore_wait(barrier, N_DEV - 1)

            @pl.when(me != 0)
            def _():
                for h in range(2):
                    rdma(0, h, me, m_send[0]).start()

        for j in range(1, 4):
            @pl.when(me != j)
            def _():
                for h in range(2):
                    rdma(j, h, me, m_send[j]).start()

        low = me < 2
        my_idx = jnp.where(low, idx_a, idx_b)
        my_rank = jnp.where(low, rank[0], rank[1])
        xh = jnp.where(low, xlo, xhi)
        k1, k2, k3 = (me + 1) % N_DEV, (me + 2) % N_DEV, (me + 3) % N_DEV
        m_recv = {1: words(me, k1), 2: words(me, k2), 3: words(me, k3)}
        m_sent = {1: words(k1, me), 2: words(k2, me), 3: words(k3, me)}
        ks = {1: k1, 2: k2, 3: k3}
        overflow = jnp.max(cum, axis=0, keepdims=True)[0, 0] > float(R)
        cp_rw.wait()
        sc = lax.dot_general(rwt_v[...].astype(BF16), xh, (((1,), (1,)), ((), ())), preferred_element_type=F32)
        pe = jnp.exp(sc - jnp.max(sc, axis=0, keepdims=True))
        gate_row = jnp.sum(jnp.where(sub8 == my_idx, pe, 0.0), axis=0, keepdims=True) / jnp.sum(pe, axis=0, keepdims=True)
        g_row = (my_idx >> 1).astype(F32) * float(NB) + my_rank
        pick = uj[:NB] == ui[:NB] + (me % 2) * NB
        g_col = jnp.sum(jnp.where(pick, g_row, 0.0), axis=1, keepdims=True)
        gate = jnp.sum(jnp.where(pick, gate_row, 0.0), axis=1, keepdims=True)
        c = lane1[:, :3 * R]
        tgt3 = jnp.where(c < R, me * NB + c, jnp.where(c < 2 * R, k1 * NB + c - R, k3 * NB + c - 2 * R)).astype(F32)
        pt3 = (g_col == tgt3).astype(BF16)
        pt_last = (g_col == (k2 * NB + lane1[:, :R]).astype(F32)).astype(BF16)
        xm = x_v[pl.ds(pl.multiple_of(me * NB, NB), NB), :].astype(BF16)
        cp_sw.wait()
        acc_v[...] = _dot(xm, sw_v[...].astype(BF16))

        @pl.when(overflow)
        def _():
            pps = []
            for t in range(2):
                st = jnp.where(mine[t] & (rank[t] >= R),
                               rank[t] - float(R) + jnp.where(second[t], float(2 * R), 0.0) + jnp.where(hi, float(R), 0.0), -1.0)
                pps.append((row_f == st).astype(BF16))
            c01 = _dot(pps[0], xlo).astype(BF16)
            c23 = _dot(pps[1], xhi).astype(BF16)
            oa = jnp.concatenate([c01[:2 * R], c23[:2 * R]], axis=0)
            ob = jnp.concatenate([c01[2 * R:], c23[2 * R:]], axis=0)
            for h in range(2):
                y = (_dot(oa, ew_v[h, 0].astype(BF16)) + _dot(ob, ew_v[h, 1].astype(BF16))).astype(BF16)
                for j in range(N_DEV):
                    ybuf1[j, :, h * HH:(h + 1) * HH] = y[j * R:(j + 1) * R]
            for j in range(N_DEV):
                @pl.when(me != j)
                def _():
                    rdma1(j, me).start()
            rbuf1[me] = ybuf1[me]
            for k in (k1, k2, k3):
                rdma1(k, k).wait_recv()
            tgt = ((lane1 >> 5) * NB + (lane1 & (R - 1)) + R).astype(F32)
            ptf = (g_col == tgt).astype(BF16)
            yall = jnp.concatenate([rbuf1[k] for k in range(N_DEV)], axis=0)
            acc_v[...] += gate * _dot(ptf, yall)
            for k in (k1, k2, k3):
                rdma1(k, k).wait_send()

        def received(d, h):
            return pltpu.bitcast(jnp.where(sub16 < m_recv[d], rbuf[ks[d], h], jnp.uint32(0)), BF16)

        for d in (1, 3):
            for h in range(2):
                rdma(ks[d], h, ks[d], m_recv[d]).wait_recv()
        base = []
        for h in range(2):
            y3 = jnp.concatenate([pltpu.bitcast(ybuf[me, h], BF16), received(1, h), received(3, h)], axis=0)
            base.append(acc_v[:, h * HH:(h + 1) * HH] + gate * _dot(pt3, y3))
        for d in (1, 2, 3):
            for h in range(2):
                rdma(ks[d], h, ks[d], m_sent[d]).wait_send()
        for h in range(2):
            rdma(k2, h, k2, m_recv[2]).wait_recv()
            yl = received(2, h)
            for m in range(4):
                sl = slice(m * 16, (m + 1) * 16)
                out_ref[sl, h * HH:(h + 1) * HH] = base[h][sl] + gate[sl] * _dot(pt_last[sl], yl)

    return pl.pallas_call(
        body,
        out_shape=jax.ShapeDtypeStruct((NB, H), F32),
        in_specs=[pl.BlockSpec(memory_space=pl.ANY)] * 5,
        out_specs=pl.BlockSpec(memory_space=pltpu.VMEM),
        scratch_shapes=[
            pltpu.VMEM((N, D), F32),
            pltpu.VMEM((E, D), F32),
            pltpu.VMEM((2, 128), I32),
            pltpu.VMEM((2, 2, D, HH), F32),
            pltpu.VMEM((D, H), F32),
            pltpu.VMEM((NB, H), F32),
            pltpu.VMEM((N_DEV, 2, RW, HH), U32),
            pltpu.VMEM((N_DEV, 2, RW, HH), U32),
            pltpu.VMEM((N_DEV, R, H), BF16),
            pltpu.VMEM((N_DEV, R, H), BF16),
            pltpu.SemaphoreType.DMA((7,)),
            pltpu.SemaphoreType.DMA((12,)),
            pltpu.SemaphoreType.DMA((12,)),
        ],
        compiler_params=pltpu.CompilerParams(collective_id=0, disable_bounds_checks=True, disable_semaphore_checks=True),
    )(x, router_W.T, route_idx.reshape(2, 128), expert_W, shared_W)
```

```python
import jax
import jax.numpy as jnp
from jax import lax
from jax.experimental import pallas as pl
from jax.experimental.pallas import tpu as pltpu

N_DEV = 4
N, D, H, E = 256, 128, 256, 8
NB = N // N_DEV
R = 32
RW = R // 2
HH = H // 2
F32, BF16, I32, U32 = jnp.float32, jnp.bfloat16, jnp.int32, jnp.uint32
LATE = 2


def _dot(a, b):
    return jnp.dot(a, b, preferred_element_type=F32)


def pallas_dist_moe_shared_ep_outshard_n256_d128_e2_h256_kernel(x, router_W, route_idx, expert_W, shared_W):
    def body(x_hbm, rwt_hbm, idx_hbm, ew_hbm, sw_hbm, out_ref,
             x_v, rwt_v, idx_v, ew_v, sw_v, acc_v, ybuf, rbuf, ybuf1, rbuf1,
             lsem, send_sems, recv_sems, go_sem):
        cp_idx = pltpu.make_async_copy(idx_hbm, idx_v, lsem.at[0])
        cp_x0 = pltpu.make_async_copy(x_hbm.at[pl.ds(0, NB)], x_v.at[pl.ds(0, NB)], lsem.at[1])
        cp_w = [pltpu.make_async_copy(ew_hbm.at[:, :, pl.ds(h * HH, HH)], ew_v.at[h], lsem.at[2 + h])
                for h in range(2)]
        cp_xr = pltpu.make_async_copy(x_hbm.at[pl.ds(NB, N - NB)], x_v.at[pl.ds(NB, N - NB)], lsem.at[4])
        cp_sw = pltpu.make_async_copy(sw_hbm, sw_v, lsem.at[5])
        cp_rw = pltpu.make_async_copy(rwt_hbm, rwt_v, lsem.at[6])
        cp_idx.start()
        cp_x0.start()
        cp_w[0].start()
        cp_w[1].start()

        me = lax.axis_index("i")
        barrier = pltpu.get_barrier_semaphore()

        def signal(sem, j):
            pl.semaphore_signal(sem, inc=1, device_id=(j,), device_id_type=pl.DeviceIdType.MESH)

        @pl.when(me != LATE)
        def _():
            signal(barrier, LATE)

        @pl.when(me == 0)
        def _():
            signal(barrier, 1)
            signal(barrier, 3)

        cp_xr.start()
        cp_sw.start()
        cp_rw.start()

        @pl.when(me == LATE)
        def _():
            pl.semaphore_wait(barrier, N_DEV - 1)
            for j in (0, 1, 3):
                signal(go_sem, j)

        def rdma(j, h, slot, m):
            return pltpu.make_async_remote_copy(
                src_ref=ybuf.at[j, h, pl.ds(0, m)], dst_ref=rbuf.at[slot, h, pl.ds(0, m)],
                send_sem=send_sems.at[2 * j + h], recv_sem=recv_sems.at[2 * slot + h],
                device_id=(j,), device_id_type=pl.DeviceIdType.MESH)

        def rdma1(j, slot):
            return pltpu.make_async_remote_copy(
                src_ref=ybuf1.at[j], dst_ref=rbuf1.at[slot],
                send_sem=send_sems.at[8 + j], recv_sem=recv_sems.at[8 + slot],
                device_id=(j,), device_id_type=pl.DeviceIdType.MESH)

        ui = lax.broadcasted_iota(I32, (128, 128), 0)
        uj = lax.broadcasted_iota(I32, (128, 128), 1)
        tri = (((ui < uj) & ((ui ^ uj) < NB)) | (uj == 0)).astype(BF16)
        sub8 = lax.broadcasted_iota(I32, (8, 128), 0)
        sub16 = ui[:16]
        lane1 = lax.broadcasted_iota(I32, (1, 128), 1)
        hi = lane1 >= NB
        row_f = ui.astype(F32)

        cp_idx.wait()
        idx_a = idx_v[0:1, :]
        idx_b = idx_v[1:2, :]
        idx16 = jnp.where(sub16 < 8, idx_a, idx_b)
        oh = ((idx16 >> 1) == (sub16 & 3)) & (hi == ((sub16 & 4) != 0))
        cum = _dot(oh.astype(BF16), tri)
        rk = jnp.where(oh & (lane1 > 0), cum, 0.0)
        rank = [jnp.sum(rk[0:8], axis=0, keepdims=True), jnp.sum(rk[8:16], axis=0, keepdims=True)]
        idxs = [idx_a, idx_b]
        mine = [(t >> 1) == me for t in idxs]
        second = [(t & 1) == 1 for t in idxs]

        def words(b, c):
            n = jnp.sum(jnp.where(sub16 == 4 * b + c, cum, 0.0), axis=0, keepdims=True).astype(I32)
            return jnp.clip((n[0, 0] + 1) >> 1, 1, RW)

        s0 = jnp.where(mine[0] & (rank[0] < R), rank[0] + jnp.where(second[0], float(R), 0.0), -1.0)
        pp0 = (row_f[:2 * R, :NB] == s0[:, :NB]).astype(BF16)
        cp_x0.wait()
        x0 = x_v[0:NB, :].astype(BF16)
        xq = [_dot(pp0[q * 16:(q + 1) * 16], x0).astype(BF16) for q in range(4)]
        m_send = [words(j, me) for j in range(N_DEV)]

        @pl.when((me & 1) == 1)
        def _():
            pl.semaphore_wait(barrier, 1)

        ws = []
        for h in range(2):
            cp_w[h].wait()
            ws.append((ew_v[h, 0].astype(BF16), ew_v[h, 1].astype(BF16)))
            for q in range(2):
                yq = (_dot(xq[q], ws[h][0]) + _dot(xq[2 + q], ws[h][1])).astype(BF16)
                ybuf[0, h, q * 8:(q + 1) * 8, :] = pltpu.bitcast(yq, U32)

            @pl.when(me != 0)
            def _():
                rdma(0, h, me, m_send[0]).start()

        pp1 = (row_f[:2 * R] == jnp.where(hi, s0, -1.0)).astype(BF16)
        s1 = jnp.where(mine[1] & (rank[1] < R),
                       rank[1] + jnp.where(second[1], float(2 * R), 0.0) + jnp.where(hi, float(R), 0.0), -1.0)
        pp23 = (row_f == s1).astype(BF16)
        cp_xr.wait()
        xlo = x_v[0:128, :].astype(BF16)
        xhi = x_v[128:256, :].astype(BF16)
        xc1 = _dot(pp1, xlo).astype(BF16)
        xc23 = _dot(pp23, xhi).astype(BF16)
        xa = jnp.concatenate([xc1[:R], xc23[:2 * R]], axis=0)
        xb = jnp.concatenate([xc1[R:], xc23[2 * R:]], axis=0)
        for h in range(2):
            y = pltpu.bitcast((_dot(xa, ws[h][0]) + _dot(xb, ws[h][1])).astype(BF16), U32)
            for j in range(1, N_DEV):
                ybuf[j, h] = y[(j - 1) * RW:j * RW]

        @pl.when(me != 0)
        def _():
            @pl.when(me != LATE)
            def _():
                pl.semaphore_wait(go_sem, 1)

            for j in range(1, N_DEV):
                @pl.when(me != j)
                def _():
                    for h in range(2):
                        rdma(j, h, me, m_send[j]).start()

        low = me < 2
        my_idx = jnp.where(low, idx_a, idx_b)
        my_rank = jnp.where(low, rank[0], rank[1])
        xh = jnp.where(low, xlo, xhi)
        k1, k2, k3 = (me + 1) % N_DEV, (me + 2) % N_DEV, (me + 3) % N_DEV
        ks = {1: k1, 2: k2, 3: k3}
        m_recv = {d: words(me, k) for d, k in ks.items()}
        m_sent = {d: words(k, me) for d, k in ks.items()}
        overflow = jnp.max(cum, axis=0, keepdims=True)[0, 0] > float(R)
        cp_rw.wait()
        sc = lax.dot_general(rwt_v[...].astype(BF16), xh, (((1,), (1,)), ((), ())),
                             preferred_element_type=F32)
        pe = jnp.exp(sc - jnp.max(sc, axis=0, keepdims=True))
        gate_row = (jnp.sum(jnp.where(sub8 == my_idx, pe, 0.0), axis=0, keepdims=True)
                    / jnp.sum(pe, axis=0, keepdims=True))
        g_row = (my_idx >> 1).astype(F32) * float(NB) + my_rank
        pick = uj[:NB] == ui[:NB] + (me % 2) * NB
        g_col = jnp.sum(jnp.where(pick, g_row, 0.0), axis=1, keepdims=True)
        gate = jnp.sum(jnp.where(pick, gate_row, 0.0), axis=1, keepdims=True)
        c = lane1[:, :3 * R]
        tgt3 = jnp.where(c < R, me * NB + c,
                         jnp.where(c < 2 * R, k1 * NB + c - R, k3 * NB + c - 2 * R)).astype(F32)
        pt3 = (g_col == tgt3).astype(BF16)
        pt_last = (g_col == (k2 * NB + lane1[:, :R]).astype(F32)).astype(BF16)
        xm = x_v[pl.ds(pl.multiple_of(me * NB, NB), NB), :].astype(BF16)
        cp_sw.wait()
        acc_v[...] = _dot(xm, sw_v[...].astype(BF16))

        @pl.when(me == 0)
        def _():
            pl.semaphore_wait(go_sem, 1)
            for j in (2, 1, 3):
                for h in range(2):
                    rdma(j, h, me, m_send[j]).start()

        @pl.when(overflow)
        def _():
            pps = []
            for t in range(2):
                st = jnp.where(mine[t] & (rank[t] >= R),
                               rank[t] - float(R) + jnp.where(second[t], float(2 * R), 0.0)
                               + jnp.where(hi, float(R), 0.0), -1.0)
                pps.append((row_f == st).astype(BF16))
            c01 = _dot(pps[0], xlo).astype(BF16)
            c23 = _dot(pps[1], xhi).astype(BF16)
            oa = jnp.concatenate([c01[:2 * R], c23[:2 * R]], axis=0)
            ob = jnp.concatenate([c01[2 * R:], c23[2 * R:]], axis=0)
            for h in range(2):
                y = (_dot(oa, ew_v[h, 0].astype(BF16)) + _dot(ob, ew_v[h, 1].astype(BF16))).astype(BF16)
                for j in range(N_DEV):
                    ybuf1[j, :, h * HH:(h + 1) * HH] = y[j * R:(j + 1) * R]
            for j in range(N_DEV):
                @pl.when(me != j)
                def _():
                    rdma1(j, me).start()
            rbuf1[me] = ybuf1[me]
            for k in (k1, k2, k3):
                rdma1(k, k).wait_recv()
            tgt = ((lane1 >> 5) * NB + (lane1 & (R - 1)) + R).astype(F32)
            ptf = (g_col == tgt).astype(BF16)
            yall = jnp.concatenate([rbuf1[k] for k in range(N_DEV)], axis=0)
            acc_v[...] += gate * _dot(ptf, yall)
            for k in (k1, k2, k3):
                rdma1(k, k).wait_send()

        def received(d, h):
            return pltpu.bitcast(jnp.where(sub16 < m_recv[d], rbuf[ks[d], h], jnp.uint32(0)), BF16)

        for d in (1, 3):
            for h in range(2):
                rdma(ks[d], h, ks[d], m_recv[d]).wait_recv()
        base = []
        for h in range(2):
            y3 = jnp.concatenate([pltpu.bitcast(ybuf[me, h], BF16), received(1, h), received(3, h)], axis=0)
            e3 = jnp.concatenate([_dot(pt3[:R], y3), _dot(pt3[R:], y3)], axis=0)
            base.append(acc_v[:, h * HH:(h + 1) * HH] + gate * e3)
        for d in (1, 2, 3):
            for h in range(2):
                rdma(ks[d], h, ks[d], m_sent[d]).wait_send()
        for h in range(2):
            rdma(k2, h, k2, m_recv[2]).wait_recv()
            yl = received(2, h)
            for m in range(4):
                sl = slice(m * 16, (m + 1) * 16)
                out_ref[sl, h * HH:(h + 1) * HH] = base[h][sl] + gate[sl] * _dot(pt_last[sl], yl)

    return pl.pallas_call(
        body,
        out_shape=jax.ShapeDtypeStruct((NB, H), F32),
        in_specs=[pl.BlockSpec(memory_space=pl.ANY)] * 5,
        out_specs=pl.BlockSpec(memory_space=pltpu.VMEM),
        scratch_shapes=[
            pltpu.VMEM((N, D), F32),
            pltpu.VMEM((E, D), F32),
            pltpu.VMEM((2, 128), I32),
            pltpu.VMEM((2, 2, D, HH), F32),
            pltpu.VMEM((D, H), F32),
            pltpu.VMEM((NB, H), F32),
            pltpu.VMEM((N_DEV, 2, RW, HH), U32),
            pltpu.VMEM((N_DEV, 2, RW, HH), U32),
            pltpu.VMEM((N_DEV, R, H), BF16),
            pltpu.VMEM((N_DEV, R, H), BF16),
            pltpu.SemaphoreType.DMA((7,)),
            pltpu.SemaphoreType.DMA((12,)),
            pltpu.SemaphoreType.DMA((12,)),
            pltpu.SemaphoreType.REGULAR,
        ],
        compiler_params=pltpu.CompilerParams(
            collective_id=0, disable_bounds_checks=True, disable_semaphore_checks=True),
    )(x, router_W.T, route_idx.reshape(2, 128), expert_W, shared_W)
```
